```python
import numpy as np

kernel_name = "dist_mlpseq_tp2d_cs_cs_b64_d2048_h4096"

def setup_inputs():
    x = np.random.randn(64, 4096).astype(np.float32)
    Win0 = np.random.randn(4096, 8192).astype(np.float32)
    Wout0 = np.random.randn(8192, 4096).astype(np.float32)
    Win1 = np.random.randn(4096, 8192).astype(np.float32)
    Wout1 = np.random.randn(8192, 4096).astype(np.float32)
    Win2 = np.random.randn(4096, 8192).astype(np.float32)
    Wout2 = np.random.randn(8192, 4096).astype(np.float32)
    return {"x": x, "Win0": Win0, "Wout0": Wout0, "Win1": Win1, "Wout1": Wout1, "Win2": Win2, "Wout2": Wout2}

def reference(x, Win0, Win1, Win2, Wout0, Wout1, Wout2):
    h = x @ Win0
    h = np.maximum(h, 0.0)
    x = h @ Wout0
    h = x @ Win1
    h = np.maximum(h, 0.0)
    x = h @ Wout1
    h = x @ Win2
    h = np.maximum(h, 0.0)
    x = h @ Wout2
    return x
```

```python
import jax
import jax.numpy as jnp
from jax import lax
from jax.experimental import pallas as pl
from jax.experimental.pallas import tpu as pltpu

B = 64
D = 2048
H = 4096
MESH = pl.DeviceIdType.MESH
BF16 = jnp.bfloat16
F32 = jnp.float32


def make(wa=(8, 8, 8, 8), wb=(7, 7, 2), tail=((8, 1), (4, 2), (2, 4), (1, 8), (1, 8)),
         lead=3, ns=8, last_split=2, mul=1):
    def kernel(x, Win0, Wout0, Win1, Wout1, Win2, Wout2):
        def body(x_hbm, a0, b0, a1, b1, a2, b2, o_ref,
                 bufa, bufb, xin, xb, hb, acch, accx, hs, hr, xs, xr,
                 wsem, tsem, xsem, ssem, rsem, tssem, trsem):
            mx, my = lax.axis_index("x"), lax.axis_index("y")
            xpeer, ypeer = (1 - mx, my), (mx, 1 - my)
            ws = (a0, b0, a1, b1, a2, b2)
            bufs = (bufa, bufb)

            def issue(p, g):
                m, half = divmod(p, 2)
                w, buf = ws[m], bufs[m % 2]
                rows = w.shape[0] // 2
                widths = (wa, wb)[m % 2]
                stride = rows // ns
                per = stride // 16
                k = 0
                for r in range(0, per, 8):
                    c = 0
                    for wd in widths:
                        for s in range(ns):
                            r0 = half * rows + ((s * mul) % ns) * stride + r + g * per
                            idx = (pl.ds(pl.multiple_of(r0, 8), 8), pl.ds(c * 128, wd * 128))
                            pltpu.make_async_copy(w.at[idx], buf.at[idx], wsem.at[p % 4]).start(priority=k % 2)
                            k += 1
                        c += wd

            def issue_loop(p, lo, hi):
                def f(g, c):
                    issue(p, g)
                    return c
                lax.fori_loop(lo, hi, f, 0)

            def wait_region(p):
                m, half = divmod(p, 2)
                buf = bufs[m % 2]
                v = buf.at[pl.ds(0, buf.shape[0] // 2), :]
                pltpu.make_async_copy(v, v, wsem.at[p % 4]).wait()

            def rdma(m, cs):
                if m % 2 == 0:
                    src, dst, dev = hs, hr, ypeer
                else:
                    src, dst, dev = xs, xr, xpeer
                l = m // 2
                return pltpu.make_async_remote_copy(
                    src.at[l, :, cs], dst.at[l, :, cs], ssem.at[m], rsem.at[m],
                    device_id=dev, device_id_type=MESH)

            def mm(lhs, buf, k0, kn, cs):
                return jnp.dot(lhs[:, pl.ds(k0, kn)], buf[pl.ds(k0, kn), cs].astype(BF16),
                               preferred_element_type=F32)

            def compute(p, j):
                m, half = divmod(p, 2)
                buf = bufs[m % 2]
                lhs, acc, snd = ((xb, acch, hs), (hb, accx, xs))[m % 2]
                rows, n = buf.shape[0] // 2, buf.shape[1] // 8
                cs = pl.ds(pl.multiple_of(j * n, 128), n)
                d = mm(lhs, buf, half * rows, rows, cs)
                if half == 0:
                    acc[:, cs] = d
                else:
                    d = d + acc[:, cs]
                    acc[:, cs] = d
                    snd[m // 2, :, cs] = d.astype(BF16)
                    rdma(m, cs).start()

            def finalize(m):
                rdma(m, slice(None)).wait_recv()
                l = m // 2
                n = 512

                def f(j, c):
                    cs = pl.ds(pl.multiple_of(j * n, 128), n)
                    if m % 2 == 0:
                        hb[:, cs] = jnp.maximum(acch[:, cs] + hr[l, :, cs].astype(F32), 0.0).astype(BF16)
                    else:
                        xb[:, cs] = (accx[:, cs] + xr[l, :, cs].astype(F32)).astype(BF16)
                    return c
                lax.fori_loop(0, (H if m % 2 == 0 else D) // n, f, 0)

            tdesc = []
            c = 0
            for t, (wd, tr) in enumerate(tail):
                nsplit = last_split if t == len(tail) - 1 else 1
                rows = (H // 2) // nsplit
                for q in range(nsplit):
                    stride = rows // ns
                    for r in range(0, stride, tr * 8):
                        for s in range(ns):
                            tdesc.append((t + q, H // 2 + q * rows + s * stride + r, tr * 8, c * 128, wd * 128))
                c += wd

            def issue_strip_step(t, c0, wd, tr, g):
                stride = (H // 2) // ns
                nsub = 32 // ns
                k = 0
                for u in range(nsub):
                    for s in range(ns):
                        r0 = H // 2 + s * stride + (g * nsub + u) * tr * 8
                        idx = (pl.ds(pl.multiple_of(r0, 8), tr * 8), pl.ds(c0, wd * 128))
                        pltpu.make_async_copy(b2.at[idx], bufb.at[idx], tsem.at[t]).start(priority=k % 2)
                        k += 1

            def issue_static(lo, hi):
                for k in range(lo, hi):
                    t, r0, nr, c0, nc = tdesc[k]
                    idx = (pl.ds(r0, nr), pl.ds(c0, nc))
                    pltpu.make_async_copy(b2.at[idx], bufb.at[idx], tsem.at[t]).start(priority=k % 2)

            def wait_strip(t, rows, n):
                v = bufb.at[pl.ds(0, rows), pl.ds(0, n)]
                pltpu.make_async_copy(v, v, tsem.at[t]).wait()

            def trdma(t, cs):
                return pltpu.make_async_remote_copy(
                    xs.at[2, :, cs], xr.at[2, :, cs], tssem.at[t], trsem.at[t],
                    device_id=xpeer, device_id_type=MESH)

            def tail_piece(t, cs, k0=H // 2, kn=H // 2, send=True):
                d = mm(hb, bufb, k0, kn, cs) + accx[:, cs]
                accx[:, cs] = d
                if send:
                    xs[2, :, cs] = d.astype(BF16)
                    trdma(t, cs).start()

            def tail_out(t, cs):
                trdma(t, cs).wait_recv()
                o_ref[:, cs] = accx[:, cs] + xr[2, :, cs].astype(F32)

            issue_loop(0, 0, 2)
            xcopy = pltpu.make_async_copy(x_hbm, xin, xsem)
            xcopy.start()
            bar = pltpu.get_barrier_semaphore()
            pl.semaphore_signal(bar, 1, device_id=xpeer, device_id_type=MESH)
            pl.semaphore_signal(bar, 1, device_id=ypeer, device_id_type=MESH)
            issue_loop(0, 2, 8)
            xcopy.wait()
            xb[...] = xin[...].astype(BF16)
            pl.semaphore_wait(bar, 2)
            issue_loop(0, 8, 16)
            for p in range(1, 11):
                issue_loop(p, 0, lead)
                if p % 2 == 1 and p > 1:
                    finalize((p - 1) // 2 - 1)
                wait_region(p - 1)

                def f(j, c, p=p):
                    issue(p, j + lead)
                    compute(p - 1, j)
                    return c
                lax.fori_loop(0, 8, f, 0)
                issue_loop(p, lead + 8, 16)

            def f(g, c):
                issue_strip_step(0, 0, 8, 1, g)
                return c
            lax.fori_loop(0, lead, f, 0)
            finalize(4)
            wait_region(10)

            n1 = 8 - lead

            def f(j, c):
                issue_strip_step(0, 0, 8, 1, j + lead)
                compute(10, j)
                return c
            lax.fori_loop(0, n1, f, 0)

            def f(j, c):
                issue_strip_step(1, 1024, 4, 2, j)
                compute(10, j + n1)
                return c
            lax.fori_loop(0, lead, f, 0)
            k = 256 + 32 * lead
            wait_strip(0, H // 2, 1024)
            for j in range(4):
                issue_static(k, k + 16)
                k += 16
                tail_piece(0, pl.ds(j * 256, 256))
            issue_static(k, 448)
            wait_strip(1, H // 2, 512)
            tail_piece(1, pl.ds(1024, 256))
            issue_static(448, 464)
            tail_piece(1, pl.ds(1280, 256))
            issue_static(464, 496)
            wait_strip(2, H // 2, 256)
            tail_piece(2, pl.ds(1536, 256))
            issue_static(496, 512)
            wait_strip(3, H // 2, 128)
            tail_piece(3, pl.ds(1792, 128))
            tail_out(0, pl.ds(0, 1024))
            for m in range(5):
                rdma(m, slice(None)).wait_send()
            rows = (H // 2) // last_split
            for q in range(last_split):
                wait_strip(4 + q, rows, 128)
                tail_piece(4, pl.ds(1920, 128), H // 2 + q * rows, rows, send=q == last_split - 1)
            tail_out(1, pl.ds(1024, 512))
            tail_out(2, pl.ds(1536, 256))
            tail_out(3, pl.ds(1792, 128))
            for t, (c0, n) in enumerate(((0, 1024), (1024, 512), (1536, 256), (1792, 128))):
                trdma(t, pl.ds(c0, n)).wait_send()
            tail_out(4, pl.ds(1920, 128))
            trdma(4, pl.ds(1920, 128)).wait_send()

        return pl.pallas_call(
            body,
            out_shape=jax.ShapeDtypeStruct((B, D), F32),
            in_specs=[pl.BlockSpec(memory_space=pltpu.HBM)] * 7,
            out_specs=pl.BlockSpec(memory_space=pltpu.VMEM),
            scratch_shapes=[
                pltpu.VMEM((D, H), F32), pltpu.VMEM((H, D), F32),
                pltpu.VMEM((B, D), F32), pltpu.VMEM((B, D), BF16), pltpu.VMEM((B, H), BF16),
                pltpu.VMEM((B, H), F32), pltpu.VMEM((B, D), F32),
                pltpu.VMEM((3, B, H), BF16), pltpu.VMEM((3, B, H), BF16),
                pltpu.VMEM((3, B, D), BF16), pltpu.VMEM((3, B, D), BF16),
                pltpu.SemaphoreType.DMA((4,)), pltpu.SemaphoreType.DMA((4 + last_split,)),
                pltpu.SemaphoreType.DMA,
                pltpu.SemaphoreType.DMA((5,)), pltpu.SemaphoreType.DMA((5,)),
                pltpu.SemaphoreType.DMA((5,)), pltpu.SemaphoreType.DMA((5,)),
            ],
            compiler_params=pltpu.CompilerParams(
                vmem_limit_bytes=100 << 20, disable_bounds_checks=True, collective_id=0),
        )(x, Win0, Wout0, Win1, Wout1, Win2, Wout2)
    return kernel


pallas_dist_mlpseq_tp2d_cs_cs_b64_d2048_h4096_kernel = make()
```

```python
import contextlib

import jax
import jax.numpy as jnp
from jax import lax
from jax.experimental import pallas as pl
from jax.experimental.pallas import tpu as pltpu

B = 64
D = 2048
H = 4096
MESH = pl.DeviceIdType.MESH
BF16 = jnp.bfloat16
F32 = jnp.float32


def nat(widths, ns=8, order=None):
    ds, c = [], 0
    for w in widths:
        for s in (order or range(ns)):
            ds.append((s, c, w))
        c += w
    return tuple(ds)


def make(pat=nat((6, 1, 1, 8)), stride=256, lead=6, xmode="asym", w0=((7, 1), (7, 1)), scopes=False,
         s0bits=(9, 10, 11, 4, 5, 6, 7, 8), s1=((4, 1, 7), (4, 10, 11, 5, 6, 8, 9)), s2=((1, 3, 7), (6, 10, 11, 4, 5)),
         s3=((1, 3, 7), (6, 10, 11, 4, 5)), s4=((1, 3, 8), (6, 7, 4, 5, 11)),
         tsched=(480, 496, 512, 512, 512), nosem=True, last_split=2, t0lead=3):
    scope = jax.named_scope if scopes else (lambda n: contextlib.nullcontext())
    ns = 8
    SPM = 64
    SPR = SPM // 2

    def kernel(x, Win0, Wout0, Win1, Wout1, Win2, Wout2):
        def body(x_hbm, a0, b0, a1, b1, a2, b2, o_ref,
                 bufa, bufb, xin, xb, hb, acch, accx, hs, hr, xs, xr,
                 wsem, tsem, xsem, ssem, rsem, tssem, trsem):
            mx, my = lax.axis_index("x"), lax.axis_index("y")
            xpeer, ypeer = (1 - mx, my), (mx, 1 - my)
            ws = (a0, b0, a1, b1, a2, b2)
            bufs = (bufa, bufb)

            def issue(m, g, sem):
                w, buf = ws[m], bufs[m % 2]
                tc = w.shape[1] // 128
                per = stride // 16
                t = (g // per) * (stride * ns) + (g % per) * 16
                r0 = (t // tc) * 8
                c0 = (t % tc) * 128 if tc > 16 else 0
                for k, (s, c, wd) in enumerate(pat):
                    cc = c0 + c * 128
                    idx = (pl.ds(pl.multiple_of(r0 + (s * stride // tc) * 8, 8), 8),
                           pl.ds(pl.multiple_of(cc, 128) if tc > 16 else cc, wd * 128))
                    pltpu.make_async_copy(w.at[idx], buf.at[idx], sem).start(priority=k % 2)

            def rdma(a, l, cs):
                src, dst, dev = ((hs, hr, ypeer), (xs, xr, xpeer))[a]
                return pltpu.make_async_remote_copy(
                    src.at[l, :, cs], dst.at[l, :, cs], ssem.at[2 * l + a], rsem.at[2 * l + a],
                    device_id=dev, device_id_type=MESH)

            def mm(lhs, buf, ks, cs):
                return jnp.dot(lhs[:, ks], buf[ks, cs].astype(BF16), preferred_element_type=F32)

            def compute(a, l, half, j):
                buf = bufs[a]
                lhs, acc, snd = ((xb, acch, hs), (hb, accx, xs))[a]
                rows, n = buf.shape[0] // 2, buf.shape[1] // 16
                cs = pl.ds(pl.multiple_of(j * n, 128), n)
                d = mm(lhs, buf, pl.ds(pl.multiple_of(half * rows, rows), rows), cs)

                @pl.when(half == 0)
                def _():
                    acc[:, cs] = d

                @pl.when(half == 1)
                def _():
                    e = d + acc[:, cs]
                    acc[:, cs] = e
                    snd[l, :, cs] = e.astype(BF16)
                    rdma(a, l, cs).start()

            def finalize(a, l):
                with scope(f"wrecv{a}"):
                    rdma(a, l, slice(None)).wait_recv()
                n = 512

                def f(j, c):
                    cs = pl.ds(pl.multiple_of(j * n, 128), n)
                    if a == 0:
                        hb[:, cs] = jnp.maximum(acch[:, cs] + hr[l, :, cs].astype(F32), 0.0).astype(BF16)
                    else:
                        xb[:, cs] = (accx[:, cs] + xr[l, :, cs].astype(F32)).astype(BF16)
                    return c
                lax.fori_loop(0, (H, D)[a] // n, f, 0)

            def tile_copy(t, spec, col, addr, k):
                wd, nb, sp = spec
                if nb == 0:
                    r = H // 2 + (addr >> 4) * 8
                    if not isinstance(r, int):
                        r = pl.multiple_of(r, 8)
                    idx = (pl.ds(r, 8), pl.ds(col * 128, wd * 128))
                    src, dst = b2.at[idx], bufb.at[idx]
                else:
                    rows = 8 << (sp - 4)
                    shp = (H // rows, rows, D)
                    i0 = (H // 2) // rows + (addr >> sp)
                    r = ((addr & ((1 << sp) - 1)) >> 4) * 8
                    if not isinstance(r, int):
                        r = pl.multiple_of(r, 8)
                    idx = (pl.ds(i0, 1 << nb), pl.ds(r, 8), pl.ds(col * 128, wd * 128))
                    src, dst = b2.reshape(shp).at[idx], bufb.reshape(shp).at[idx]
                pltpu.make_async_copy(src, dst, tsem.at[t]).start(priority=k % 2)

            def deposit(i, bits):
                a = 0
                for j, b in enumerate(bits):
                    a = a + (((i >> j) & 1) << b)
                return a

            def issue_strip0(g):
                base = deposit(g, s0bits[4:])
                k = 0
                for u in range(2):
                    c = 0
                    for wd in w0[u]:
                        for s in range(8):
                            tile_copy(0, (wd, 0, 0), c, base + deposit(u * 8 + s, s0bits[:4]), k)
                            k += 1
                        c += wd

            def issue_strip1(g):
                spec, bits = s1
                base = deposit(g, bits[4:])
                for k in range(16):
                    tile_copy(1, spec, 8, base + deposit(k, bits[:4]), k)

            tdesc = [None] * 256
            for i in range(128):
                tdesc.append((1, s1[0], 8, deposit(i, s1[1])))
            for i in range(64):
                if s2[0][0] == 2:
                    tdesc.append((2, s2[0], 12, deposit(i, s2[1])))
                else:
                    tdesc.append((2, s2[0], 12 + i // 32, deposit(i % 32, s2[1])))
            for i in range(32):
                tdesc.append((3, s3[0], 14, deposit(i, s3[1])))
            for i in range(32):
                tdesc.append((4 + i * last_split // 32, s4[0], 15, deposit(i, s4[1])))

            def issue_static(lo, hi):
                for k in range(lo, hi):
                    tile_copy(*tdesc[k], k)

            def wait_strip(t, rows, n):
                v = bufb.at[pl.ds(0, rows), pl.ds(0, n)]
                with scope(f"wstrip{t}"):
                    pltpu.make_async_copy(v, v, tsem.at[t]).wait()

            def trdma(t, cs):
                return pltpu.make_async_remote_copy(
                    xs.at[2, :, cs], xr.at[2, :, cs], tssem.at[t], trsem.at[t],
                    device_id=xpeer, device_id_type=MESH)

            def tail_piece(t, cs, k0=H // 2, kn=H // 2, send=True):
                d = mm(hb, bufb, pl.ds(k0, kn), cs) + accx[:, cs]
                accx[:, cs] = d
                if send:
                    xs[2, :, cs] = d.astype(BF16)
                    trdma(t, cs).start()

            def tail_out(t, cs):
                with scope(f"trecv{t}"):
                    trdma(t, cs).wait_recv()
                o_ref[:, cs] = accx[:, cs] + xr[2, :, cs].astype(F32)

            bar = pltpu.get_barrier_semaphore()
            xfull = pltpu.make_async_copy(x_hbm, xin, xsem.at[0])
            xsend = pltpu.make_async_remote_copy(xb, xb, xsem.at[1], xsem.at[2], device_id=xpeer, device_id_type=MESH)

            NMAIN = 5 * SPM + SPR
            T0 = 16
            nsteps = NMAIN + lead + 16

            def step(s, carry):
                m_dyn, g = s // SPM, s % SPM
                sem = wsem.at[(s // SPR) % 4]
                for m in range(6):
                    @pl.when((m_dyn == m) & (s < NMAIN))
                    def _(m=m):
                        issue(m, g, sem)

                @pl.when((s >= NMAIN) & (s < NMAIN + T0))
                def _():
                    issue_strip0(s - NMAIN)

                @pl.when(s >= NMAIN + T0)
                def _():
                    issue_strip1(s - NMAIN - T0)

                @pl.when(s == 3)
                def _():
                    if xmode == "full":
                        xfull.start()
                    else:
                        @pl.when(mx == 0)
                        def _():
                            xfull.start()
                    pl.semaphore_signal(bar, 1, device_id=xpeer, device_id_type=MESH)
                    pl.semaphore_signal(bar, 1, device_id=ypeer, device_id_type=MESH)

                @pl.when(s == 12)
                def _():
                    pl.semaphore_wait(bar, 2)
                    if xmode == "full":
                        xfull.wait()
                        xb[...] = xin[...].astype(BF16)
                    else:
                        @pl.when(mx == 0)
                        def _():
                            xfull.wait()
                            xb[...] = xin[...].astype(BF16)
                            xsend.start()

                if xmode != "full":
                    @pl.when(s == 30)
                    def _():
                        @pl.when(mx == 0)
                        def _():
                            xsend.wait_send()

                        @pl.when(mx == 1)
                        def _():
                            xsend.wait_recv()

                c = s - SPR - lead
                q, j = c // SPR, c % SPR

                @pl.when((c >= 0) & (j < 16))
                def _():
                    l, a, half = q // 4, (q // 2) % 2, q % 2

                    @pl.when(j == 0)
                    def _():
                        @pl.when(q % 4 == 2)
                        def _():
                            finalize(0, l)

                        @pl.when((q % 4 == 0) & (q > 0))
                        def _():
                            finalize(1, l - 1)
                        v = bufa.at[pl.ds(0, D // 2), :]
                        with scope("wreg"):
                            pltpu.make_async_copy(v, v, wsem.at[q % 4]).wait()

                    @pl.when(a == 0)
                    def _():
                        compute(0, l, half, j)

                    @pl.when(a == 1)
                    def _():
                        compute(1, l, half, j)
                return carry

            lax.fori_loop(0, nsteps, step, 0)
            k = 256 + 16 * lead
            wait_strip(0, H // 2, 1024)
            k1 = 384

            if k < k1:
                def f(j, c):
                    issue_strip1(lead + j)
                    tail_piece(0, pl.ds(pl.multiple_of(j * 256, 128), 256))
                    return c
                lax.fori_loop(0, (k1 - k) // 16, f, 0)
            done = max(0, (k1 - k) // 16)
            k = max(k, k1)
            for j in range(done, 4):
                tail_piece(0, pl.ds(j * 256, 256))
                issue_static(k, k + 16)
                k += 16
            for m in range(5):
                rdma(m % 2, m // 2, slice(None)).wait_send()
            issue_static(k, tsched[0])
            wait_strip(1, H // 2, 512)
            tail_piece(1, pl.ds(1024, 256))
            issue_static(tsched[0], tsched[1])
            tail_piece(1, pl.ds(1280, 256))
            issue_static(tsched[1], tsched[2])
            wait_strip(2, H // 2, 256)
            tail_piece(2, pl.ds(1536, 256))
            issue_static(tsched[2], tsched[4])
            wait_strip(3, H // 2, 128)
            tail_piece(3, pl.ds(1792, 128))
            rows = (H // 2) // last_split
            for q in range(last_split):
                wait_strip(4 + q, rows, 128)
                tail_piece(4, pl.ds(1920, 128), H // 2 + q * rows, rows, send=q == last_split - 1)
            tail_out(0, pl.ds(0, 1024))
            tail_out(1, pl.ds(1024, 512))
            tail_out(2, pl.ds(1536, 256))
            tail_out(3, pl.ds(1792, 128))
            for t, (c0, n) in enumerate(((0, 1024), (1024, 512), (1536, 256), (1792, 128))):
                trdma(t, pl.ds(c0, n)).wait_send()
            tail_out(4, pl.ds(1920, 128))
            with scope("lastsend"):
                trdma(4, pl.ds(1920, 128)).wait_send()

        return pl.pallas_call(
            body,
            out_shape=jax.ShapeDtypeStruct((B, D), F32),
            in_specs=[pl.BlockSpec(memory_space=pltpu.HBM)] * 7,
            out_specs=pl.BlockSpec(memory_space=pltpu.VMEM),
            scratch_shapes=[
                pltpu.VMEM((D, H), F32), pltpu.VMEM((H, D), F32),
                pltpu.VMEM((B, D), F32), pltpu.VMEM((B, D), BF16), pltpu.VMEM((B, H), BF16),
                pltpu.VMEM((B, H), F32), pltpu.VMEM((B, D), F32),
                pltpu.VMEM((3, B, H), BF16), pltpu.VMEM((3, B, H), BF16),
                pltpu.VMEM((3, B, D), BF16), pltpu.VMEM((3, B, D), BF16),
                pltpu.SemaphoreType.DMA((4,)), pltpu.SemaphoreType.DMA((4 + last_split,)),
                pltpu.SemaphoreType.DMA((3,)),
                pltpu.SemaphoreType.DMA((5,)), pltpu.SemaphoreType.DMA((5,)),
                pltpu.SemaphoreType.DMA((5,)), pltpu.SemaphoreType.DMA((5,)),
            ],
            compiler_params=pltpu.CompilerParams(
                vmem_limit_bytes=100 << 20, disable_bounds_checks=True, collective_id=0,
                disable_semaphore_checks=nosem),
        )(x, Win0, Wout0, Win1, Wout1, Win2, Wout2)
    return kernel


pallas_dist_mlpseq_tp2d_cs_cs_b64_d2048_h4096_kernel = make()
```

```python
import contextlib

import jax
import jax.numpy as jnp
from jax import lax
from jax.experimental import pallas as pl
from jax.experimental.pallas import tpu as pltpu

B = 64
D = 2048
H = 4096
MESH = pl.DeviceIdType.MESH
BF16 = jnp.bfloat16
F32 = jnp.float32


def deposit(i, bits):
    a = 0
    for j, b in enumerate(bits):
        a = a + (((i >> j) & 1) << b)
    return a


def make(mbits=(5, 6, 7, 0, 1, 2, 3, 4), lead=4, scopes=False,
         s0bits=(9, 10, 11, 4, 5, 6, 7, 8), s1=((4, 1, 7), (4, 10, 11, 5, 6, 8, 9)),
         s2=((1, 3, 7), (6, 10, 11, 4, 5)), s3=((1, 3, 7), (6, 10, 11, 4, 5)), s4=((1, 3, 8), (6, 7, 4, 5, 11)),
         cols=(7, 3, 1, 0, 15), tsched=(480, 496, 512), split=(1024, 1024), compact=True):
    scope = jax.named_scope if scopes else (lambda n: contextlib.nullcontext())
    SPM = 64
    SPR = SPM // 2
    widths = (8, 4, 2, 1, 1)

    def kernel(x, Win0, Wout0, Win1, Wout1, Win2, Wout2):
        def body(x_hbm, a0, b0, a1, b1, a2, b2, o_ref,
                 bufa, bufb, bufl, xin, xb, hb, acch, accx, hs, hr, xs, xr,
                 wsem, tsem, xsem, ssem, rsem, tssem, trsem):
            mx, my = lax.axis_index("x"), lax.axis_index("y")
            xpeer, ypeer = (1 - mx, my), (mx, 1 - my)
            ws = (a0, b0, a1, b1, a2, b2)
            bufs = (bufa, bufb)

            def issue(m, half, g, sem):
                w, buf = ws[m], bufs[m % 2]
                base = deposit(g, mbits[3:])
                for i in range(0, 8, 2):
                    for part in range(2):
                        for t in range(2):
                            blk = ((base + deposit(i + t, mbits[:3]) + part) & 255) + half * 256
                            c, wd = ((7, 9), (0, 7))[part]
                            if m % 2 == 0:
                                idx = (pl.ds(pl.multiple_of((blk >> 1) * 8, 8), 8),
                                       pl.ds(pl.multiple_of(((blk & 1) * 16 + c) * 128, 128), wd * 128))
                            else:
                                idx = (pl.ds(pl.multiple_of(blk * 8, 8), 8), pl.ds(c * 128, wd * 128))
                            pltpu.make_async_copy(w.at[idx], buf.at[idx], sem).start(priority=t)

            def rdma(a, l, cs):
                src, dst, dev = ((hs, hr, ypeer), (xs, xr, xpeer))[a]
                return pltpu.make_async_remote_copy(
                    src.at[l, :, cs], dst.at[l, :, cs], ssem.at[2 * l + a], rsem.at[2 * l + a],
                    device_id=dev, device_id_type=MESH)

            def mm(lhs, w):
                return jnp.dot(lhs, w.astype(BF16), preferred_element_type=F32)

            def compute(a, l, half, j):
                buf = bufs[a]
                lhs, acc, snd = ((xb, acch, hs), (hb, accx, xs))[a]
                rows, n = buf.shape[0] // 2, buf.shape[1] // 16
                cs = pl.ds(pl.multiple_of(j * n, 128), n)
                ks = pl.ds(pl.multiple_of(half * rows, rows), rows)
                d = mm(lhs[:, ks], buf[ks, cs])

                @pl.when(half == 0)
                def _():
                    acc[:, cs] = d

                @pl.when(half == 1)
                def _():
                    e = d + acc[:, cs]
                    acc[:, cs] = e
                    snd[l, :, cs] = e.astype(BF16)
                    rdma(a, l, cs).start()

            def finalize(a, l):
                with scope(f"wrecv{a}"):
                    rdma(a, l, slice(None)).wait_recv()
                n = 512

                def f(j, c):
                    cs = pl.ds(pl.multiple_of(j * n, 128), n)
                    if a == 0:
                        hb[:, cs] = jnp.maximum(acch[:, cs] + hr[l, :, cs].astype(F32), 0.0).astype(BF16)
                    else:
                        xb[:, cs] = (accx[:, cs] + xr[l, :, cs].astype(F32)).astype(BF16)
                    return c
                lax.fori_loop(0, (H, D)[a] // n, f, 0)

            def tile_copy(t, spec, col, addr, k):
                wd, nb, sp = spec
                if nb == 0:
                    r = H // 2 + (addr >> 4) * 8
                    if not isinstance(r, int):
                        r = pl.multiple_of(r, 8)
                    idx = (pl.ds(r, 8), pl.ds(col * 128, wd * 128))
                    src, dst = b2.at[idx], bufb.at[idx]
                else:
                    rows = 8 << (sp - 4)
                    shp = (H // rows, rows, D)
                    i0 = addr >> sp
                    r = ((addr & ((1 << sp) - 1)) >> 4) * 8
                    if not isinstance(r, int):
                        r = pl.multiple_of(r, 8)
                    idx = (pl.ds((H // 2) // rows + i0, 1 << nb), pl.ds(r, 8), pl.ds(col * 128, wd * 128))
                    src = b2.reshape(shp).at[idx]
                    if compact and t >= 4:
                        dst = bufl.reshape(H // 2 // rows, rows, 128).at[pl.ds(i0, 1 << nb), pl.ds(r, 8)]
                    else:
                        dst = bufb.reshape(shp).at[idx]
                pltpu.make_async_copy(src, dst, tsem.at[t]).start(priority=k % 2)

            def issue_strip0(g):
                base = deposit(g, s0bits[4:])
                for k in range(16):
                    tile_copy(0, (8, 0, 0), cols[0], base + deposit(k, s0bits[:4]), k)

            def issue_strip1(g):
                spec, bits = s1
                base = deposit(g, bits[4:])
                for k in range(16):
                    tile_copy(1, spec, cols[1], base + deposit(k, bits[:4]), k)

            tdesc = [None] * 256
            for i in range(128):
                tdesc.append((1, s1[0], cols[1], deposit(i, s1[1])))
            for i in range(64):
                if s2[0][0] == 2:
                    tdesc.append((2, s2[0], cols[2], deposit(i, s2[1])))
                else:
                    tdesc.append((2, s2[0], cols[2] + i // 32, deposit(i % 32, s2[1])))
            for i in range(32):
                tdesc.append((3, s3[0], cols[3], deposit(i, s3[1])))
            for i in range(32):
                addr = deposit(i, s4[1])
                row, q = (addr >> 4) * 8, 0
                while row >= sum(split[:q + 1]):
                    q += 1
                assert row + (8 << (s4[0][2] - 4)) * ((1 << s4[0][1]) - 1) < sum(split[:q + 1])
                tdesc.append((4 + q, s4[0], cols[4], addr))

            def issue_static(lo, hi):
                for k in range(lo, hi):
                    tile_copy(*tdesc[k], k)

            def wait_strip(t, rows, n):
                v = bufb.at[pl.ds(0, rows), pl.ds(0, n)]
                with scope(f"wstrip{t}"):
                    pltpu.make_async_copy(v, v, tsem.at[t]).wait()

            def trdma(t, cs):
                return pltpu.make_async_remote_copy(
                    xs.at[2, :, cs], xr.at[2, :, cs], tssem.at[t], trsem.at[t],
                    device_id=xpeer, device_id_type=MESH)

            def tail_piece(t, cs, k0=0, kn=H // 2, send=True):
                ks = pl.ds(H // 2 + k0, kn)
                d = mm(hb[:, ks], bufl[pl.ds(k0, kn), :] if compact and t == 4 else bufb[ks, cs]) + accx[:, cs]
                accx[:, cs] = d
                if send:
                    xs[2, :, cs] = d.astype(BF16)
                    trdma(t, cs).start()

            def strip(t):
                return pl.ds(cols[t] * 128, widths[t] * 128)

            def tail_out(t):
                cs = strip(t)
                with scope(f"trecv{t}"):
                    trdma(t, cs).wait_recv()
                o_ref[:, cs] = accx[:, cs] + xr[2, :, cs].astype(F32)

            bar = pltpu.get_barrier_semaphore()
            xfull = pltpu.make_async_copy(x_hbm, xin, xsem.at[0])
            xsend = pltpu.make_async_remote_copy(xb, xb, xsem.at[1], xsem.at[2], device_id=xpeer, device_id_type=MESH)

            NMAIN = 5 * SPM + SPR
            T0 = 16
            nsteps = NMAIN + lead + 16

            def step(s, carry):
                sem = wsem.at[(s >> 5) & 3]
                for m in range(6):
                    @pl.when(((s >> 6) == m) & (s < NMAIN))
                    def _(m=m):
                        issue(m, (s >> 5) & 1, s & 31, sem)

                @pl.when((s >= NMAIN) & (s < NMAIN + T0))
                def _():
                    issue_strip0(s - NMAIN)

                @pl.when(s >= NMAIN + T0)
                def _():
                    issue_strip1(s - NMAIN - T0)

                @pl.when(s == 3)
                def _():
                    @pl.when(mx == 0)
                    def _():
                        xfull.start()
                    pl.semaphore_signal(bar, 1, device_id=xpeer, device_id_type=MESH)
                    pl.semaphore_signal(bar, 1, device_id=ypeer, device_id_type=MESH)

                @pl.when(s == 13)
                def _():
                    pl.semaphore_wait(bar, 2)

                    @pl.when(mx == 0)
                    def _():
                        xfull.wait()
                        xb[...] = xin[...].astype(BF16)
                        xsend.start()

                @pl.when(s == 31)
                def _():
                    @pl.when(mx == 0)
                    def _():
                        xsend.wait_send()

                    @pl.when(mx == 1)
                    def _():
                        xsend.wait_recv()

                c = s - SPR - lead
                q, j = c >> 5, c & 31

                @pl.when((c >= 0) & (j < 16))
                def _():
                    l, a, half = q >> 2, (q >> 1) & 1, q & 1

                    @pl.when(j == 0)
                    def _():
                        @pl.when((q & 3) == 2)
                        def _():
                            finalize(0, l)

                        @pl.when(((q & 3) == 0) & (q > 0))
                        def _():
                            finalize(1, l - 1)
                        v = bufa.at[pl.ds(0, D // 2), :]
                        with scope("wreg"):
                            pltpu.make_async_copy(v, v, wsem.at[q & 3]).wait()

                    @pl.when(a == 0)
                    def _():
                        compute(0, l, half, j)

                    @pl.when(a == 1)
                    def _():
                        compute(1, l, half, j)
                return carry

            lax.fori_loop(0, nsteps, step, 0)
            k = 256 + 16 * lead
            k1 = 320
            if k < k1:
                def f(j, c):
                    issue_strip1(lead + j)
                    return c
                lax.fori_loop(0, (k1 - k) // 16, f, 0)
                k = k1
            wait_strip(0, H // 2, 1024)

            def f(j, c):
                @pl.when(k // 16 - 16 + j < 8)
                def _():
                    issue_strip1(k // 16 - 16 + j)
                tail_piece(0, pl.ds(pl.multiple_of(cols[0] * 128 + j * 256, 128), 256))
                return c
            lax.fori_loop(0, 4, f, 0)
            for m in range(5):
                rdma(m % 2, m // 2, slice(None)).wait_send()
            issue_static(384, tsched[0])
            wait_strip(1, H // 2, 512)
            tail_piece(1, pl.ds(cols[1] * 128, 256))
            issue_static(tsched[0], tsched[1])
            tail_piece(1, pl.ds(cols[1] * 128 + 256, 256))
            issue_static(tsched[1], tsched[2])
            wait_strip(2, H // 2, 256)
            tail_piece(2, strip(2))
            issue_static(tsched[2], 512)
            wait_strip(3, H // 2, 128)
            tail_piece(3, strip(3))
            for q, rows in enumerate(split):
                wait_strip(4 + q, rows, 128)
                tail_piece(4, strip(4), sum(split[:q]), rows, send=q == len(split) - 1)
            for t in range(4):
                tail_out(t)
            for t in range(4):
                trdma(t, strip(t)).wait_send()
            tail_out(4)
            with scope("lastsend"):
                trdma(4, strip(4)).wait_send()

        return pl.pallas_call(
            body,
            out_shape=jax.ShapeDtypeStruct((B, D), F32),
            in_specs=[pl.BlockSpec(memory_space=pltpu.HBM)] * 7,
            out_specs=pl.BlockSpec(memory_space=pltpu.VMEM),
            scratch_shapes=[
                pltpu.VMEM((D, H), F32), pltpu.VMEM((H, D), F32), pltpu.VMEM((H // 2, 128), F32),
                pltpu.VMEM((B, D), F32), pltpu.VMEM((B, D), BF16), pltpu.VMEM((B, H), BF16),
                pltpu.VMEM((B, H), F32), pltpu.VMEM((B, D), F32),
                pltpu.VMEM((3, B, H), BF16), pltpu.VMEM((3, B, H), BF16),
                pltpu.VMEM((3, B, D), BF16), pltpu.VMEM((3, B, D), BF16),
                pltpu.SemaphoreType.DMA((4,)), pltpu.SemaphoreType.DMA((4 + len(split),)),
                pltpu.SemaphoreType.DMA((3,)),
                pltpu.SemaphoreType.DMA((5,)), pltpu.SemaphoreType.DMA((5,)),
                pltpu.SemaphoreType.DMA((5,)), pltpu.SemaphoreType.DMA((5,)),
            ],
            compiler_params=pltpu.CompilerParams(
                vmem_limit_bytes=100 << 20, disable_bounds_checks=True, collective_id=0,
                disable_semaphore_checks=True),
        )(x, Win0, Wout0, Win1, Wout1, Win2, Wout2)
    return kernel


pallas_dist_mlpseq_tp2d_cs_cs_b64_d2048_h4096_kernel = make()
```

```python
import jax
import jax.numpy as jnp
from jax import lax
from jax.experimental import pallas as pl
from jax.experimental.pallas import tpu as pltpu

B, D, H = 64, 2048, 4096
LANES = 128
GROUP = 64
HALF = H // GROUP // 2

STREAMS, STEPS = 8, 32
BLOCK_COPIES = ((0, 7, 8), (0, 15, 1), (1, 0, 7))
LAG = 5
PIECES = 16

WIDE_COL, WIDE_ORDER = 7, (2, 6, 7, 0, 1, 5, 3, 4)
MID_COL, MID_ORDER = 3, (0, 6, 7, 1, 2, 4, 5)
NARROW_COLS, NARROW_ORDER = (1, 2, 0, 15), (2, 6, 7, 0, 1)
LAST_ORDER = (2, 6, 0, 1, 7)
OTHER_QUEUE = (77, 99)


def _scatter_bits(i, positions):
    return sum(((i >> j) & 1) << p for j, p in enumerate(positions))


def _tiles(first, count, size):
    start = first * size
    if not isinstance(start, int):
        start = pl.multiple_of(start, size)
    return pl.ds(start, count * size)


def _matmul(lhs, w):
    w = w.reshape(lhs.shape[1], w.shape[-1]).astype(jnp.bfloat16)
    return jnp.dot(lhs, w, preferred_element_type=jnp.float32)


def _wait_filled(dst, sem):
    pltpu.make_async_copy(dst, dst, sem).wait()


def _remote_copy(src, dst, send_sem, recv_sem, peer):
    return pltpu.make_async_remote_copy(
        src, dst, send_sem, recv_sem, device_id=peer, device_id_type=pl.DeviceIdType.MESH
    )


def _body(
    x_hbm, win0, wout0, win1, wout1, win2, wout2,
    out_ref,
    win_buf, wout_buf, wide_buf, mid_buf, narrow_buf,
    x_f32, x_lhs, h_lhs, h_acc, x_acc,
    h_send, h_recv, x_send, x_recv, narrow_send, narrow_recv,
    region_sems, mid_sem, narrow_sems, x_sems,
    send_sems, recv_sems, narrow_send_sems, narrow_recv_sems,
):
    weights = (win0, wout0, win1, wout1, win2, wout2)
    my_x, my_y = lax.axis_index("x"), lax.axis_index("y")
    x_peer, y_peer = (1 - my_x, my_y), (my_x, 1 - my_y)

    def fetch(p, step):
        m, half = divmod(p, 2)
        for pair in range(0, STREAMS, 2):
            for is_next, tile, count in BLOCK_COPIES:
                block = step + is_next
                for queue in range(2):
                    stream = pair + queue
                    wraps = stream == STREAMS - 1
                    if m % 2 == 0:
                        row = 16 * stream + (block >> 1)
                        row = row & 127 if wraps else row
                        col = 16 * (block & 1) + tile
                        at = (_tiles(128 * half + row, 1, 8), _tiles(col, count, LANES))
                    else:
                        group = 4 * stream + (block >> 3)
                        group = group & (HALF - 1) if wraps else group
                        at = (HALF * half + group, _tiles(block & 7, 1, 8), _tiles(tile, count, LANES))
                    pltpu.make_async_copy(
                        weights[m].at[at], (win_buf, wout_buf)[m % 2].at[at], region_sems.at[half]
                    ).start(priority=queue)

    def exchange(m, cols, sem):
        src, dst, peer = ((h_send, h_recv, y_peer), (x_send, x_recv, x_peer))[m % 2]
        return _remote_copy(
            src.at[m // 2, :, cols], dst.at[m // 2, :, cols], send_sems.at[sem], recv_sems.at[sem], peer
        )

    def multiply(p, piece):
        m, half = divmod(p, 2)
        lhs, acc, send = ((x_lhs, h_acc, h_send), (h_lhs, x_acc, x_send))[m % 2]
        k = lhs.shape[1] // 2
        cols = _tiles(piece, 1, acc.shape[1] // PIECES)
        if m % 2 == 0:
            w = win_buf[_tiles(half, 1, k), cols]
        else:
            w = wout_buf[_tiles(half, 1, HALF), :, cols]
        partial = _matmul(lhs[:, _tiles(half, 1, k)], w)
        if half == 0:
            acc[:, cols] = partial
        else:
            partial = partial + acc[:, cols]
            acc[:, cols] = partial
            send[m // 2, :, cols] = partial.astype(jnp.bfloat16)
            exchange(m, cols, m).start()

    def all_reduce(m):
        exchange(m, slice(None), m).wait_recv()

        @pl.loop(0, (H, D)[m % 2] // 512)
        def _(j):
            cols = _tiles(j, 1, 512)
            if m % 2 == 0:
                total = h_acc[:, cols] + h_recv[m // 2, :, cols].astype(jnp.float32)
                h_lhs[:, cols] = jnp.maximum(total, 0.0).astype(jnp.bfloat16)
            else:
                total = x_acc[:, cols] + x_recv[m // 2, :, cols].astype(jnp.float32)
                x_lhs[:, cols] = total.astype(jnp.bfloat16)

    def consume(p, step):
        m, half = divmod(p, 2)

        @pl.when(step == LAG)
        def _():
            if half == 0 and m > 0:
                all_reduce(m - 1)
            buf = (win_buf, wout_buf)[m % 2]
            _wait_filled(buf.at[_tiles(half, 1, buf.shape[0] // 2)], region_sems.at[half])

        @pl.when((step >= LAG) & (step < LAG + PIECES))
        def _():
            multiply(p, step - LAG)

    x_load = pltpu.make_async_copy(x_hbm, x_f32, x_sems.at[0])
    x_share = _remote_copy(x_lhs, x_lhs, x_sems.at[1], x_sems.at[2], x_peer)
    barrier = pltpu.get_barrier_semaphore()

    @pl.loop(0, STEPS)
    def _(step):
        fetch(0, step)

        @pl.when(step == 3)
        def _():
            pl.when(my_x == 0)(x_load.start)
            for peer in (x_peer, y_peer):
                pl.semaphore_signal(barrier, 1, device_id=peer, device_id_type=pl.DeviceIdType.MESH)

        @pl.when(step == 13)
        def _():
            pl.semaphore_wait(barrier, 2)

            @pl.when(my_x == 0)
            def _():
                x_load.wait()
                x_lhs[...] = x_f32[...].astype(jnp.bfloat16)
                x_share.start()

    pl.when(my_x == 0)(x_share.wait_send)
    pl.when(my_x == 1)(x_share.wait_recv)

    for p in range(1, 11):

        @pl.loop(0, STEPS)
        def _(step, p=p):
            fetch(p, step)
            consume(p - 1, step)

    def fetch_strip(dst, sem, col, block, queue):
        width = dst.shape[-1] // LANES
        rows = _tiles(block & 7, 1, 8)
        pltpu.make_async_copy(
            wout2.at[pl.ds(HALF + (block >> 3), 8 // width), rows, _tiles(col, width, LANES)],
            dst.at[pl.ds(block >> 3, 8 // width), rows, :],
            sem,
        ).start(priority=queue)

    def fetch_strip_step(dst, sem, col, order, step):
        first = _scatter_bits(step, order[4:])
        for i in range(16):
            fetch_strip(dst, sem, col, first + _scatter_bits(i, order[:4]), i % 2)

    def fetch_narrow(start, stop):
        for i in range(start, stop):
            strip = i // 32
            block = _scatter_bits(i % 32, LAST_ORDER if strip == 3 else NARROW_ORDER)
            sem = strip + (block >> 7 if strip == 3 else 0)
            queue = (i + (i in OTHER_QUEUE)) % 2
            fetch_strip(narrow_buf.at[strip], narrow_sems.at[sem], NARROW_COLS[strip], block, queue)

    def multiply_strip(buf, col, piece, sem):
        cols = _tiles(col + 2 * piece, 2, LANES)
        w = buf[:, :, _tiles(2 * piece, 2, LANES)]
        partial = x_acc[:, cols] + _matmul(h_lhs[:, _tiles(1, 1, H // 2)], w)
        x_acc[:, cols] = partial
        x_send[2, :, cols] = partial.astype(jnp.bfloat16)
        exchange(5, cols, sem).start()

    def exchange_narrow(strip):
        return _remote_copy(
            narrow_send.at[strip], narrow_recv.at[strip],
            narrow_send_sems.at[strip], narrow_recv_sems.at[strip], x_peer,
        )

    wide_step = LAG + PIECES

    @pl.loop(0, wide_step + 4)
    def _(step):
        @pl.when(step < 16)
        def _():
            fetch_strip_step(wide_buf, region_sems.at[1], WIDE_COL, WIDE_ORDER, step)

        @pl.when((step >= 16) & (step < 24))
        def _():
            fetch_strip_step(mid_buf, mid_sem, MID_COL, MID_ORDER, step - 16)

        consume(10, step)

        @pl.when(step == wide_step)
        def _():
            _wait_filled(wide_buf, region_sems.at[1])

        @pl.when(step >= wide_step)
        def _():
            multiply_strip(wide_buf, WIDE_COL, step - wide_step, 5)

    fetch_narrow(0, 96)
    _wait_filled(mid_buf, mid_sem)
    for piece in range(2):
        multiply_strip(mid_buf, MID_COL, piece, 6)
        fetch_narrow(96 + 16 * piece, 112 + 16 * piece)

    for strip, col in enumerate(NARROW_COLS):
        cols = _tiles(col, 1, LANES)
        partial = x_acc[:, cols]
        parts = 2 if strip == 3 else 1
        for part in range(parts):
            w = narrow_buf.at[strip, _tiles(part, 1, HALF // parts)]
            _wait_filled(w, narrow_sems.at[strip + part])
            partial = partial + _matmul(h_lhs[:, _tiles(parts + part, 1, H // 2 // parts)], w[...])
        narrow_send[strip] = partial.astype(jnp.bfloat16)
        exchange_narrow(strip).start()
        x_acc[:, cols] = partial

    for m in range(5):
        exchange(m, slice(None), m).wait_send()
    for cols, sem in ((_tiles(WIDE_COL, 8, LANES), 5), (_tiles(MID_COL, 4, LANES), 6)):
        exchange(5, cols, sem).wait()
        out_ref[:, cols] = x_acc[:, cols] + x_recv[2, :, cols].astype(jnp.float32)
    for strip, col in enumerate(NARROW_COLS):
        cols = _tiles(col, 1, LANES)
        exchange_narrow(strip).wait()
        out_ref[:, cols] = x_acc[:, cols] + narrow_recv[strip].astype(jnp.float32)


def pallas_dist_mlpseq_tp2d_cs_cs_b64_d2048_h4096_kernel(
    x: jax.Array,
    Win0: jax.Array,
    Wout0: jax.Array,
    Win1: jax.Array,
    Wout1: jax.Array,
    Win2: jax.Array,
    Wout2: jax.Array,
):
    f32, bf16 = jnp.float32, jnp.bfloat16
    grouped = (2 * HALF, GROUP, D)
    dma = pltpu.SemaphoreType.DMA
    return pl.pallas_call(
        _body,
        out_shape=jax.ShapeDtypeStruct((B, D), f32),
        in_specs=[pl.BlockSpec(memory_space=pltpu.HBM)] * 7,
        out_specs=pl.BlockSpec(memory_space=pltpu.VMEM),
        scratch_shapes=[
            pltpu.VMEM((D, H), f32),
            pltpu.VMEM(grouped, f32),
            pltpu.VMEM((HALF, GROUP, 8 * LANES), f32),
            pltpu.VMEM((HALF, GROUP, 4 * LANES), f32),
            pltpu.VMEM((4, HALF, GROUP, LANES), f32),
            pltpu.VMEM((B, D), f32),
            pltpu.VMEM((B, D), bf16),
            pltpu.VMEM((B, H), bf16),
            pltpu.VMEM((B, H), f32),
            pltpu.VMEM((B, D), f32),
            pltpu.VMEM((3, B, H), bf16),
            pltpu.VMEM((3, B, H), bf16),
            pltpu.VMEM((3, B, D), bf16),
            pltpu.VMEM((3, B, D), bf16),
            pltpu.VMEM((4, B, LANES), bf16),
            pltpu.VMEM((4, B, LANES), bf16),
            dma((2,)),
            dma,
            dma((5,)),
            dma((3,)),
            dma((7,)),
            dma((7,)),
            dma((4,)),
            dma((4,)),
        ],
        compiler_params=pltpu.CompilerParams(
            vmem_limit_bytes=100 * 1024 * 1024,
            collective_id=0,
            disable_bounds_checks=True,
            disable_semaphore_checks=True,
        ),
    )(
        x,
        Win0,
        Wout0.reshape(grouped),
        Win1,
        Wout1.reshape(grouped),
        Win2,
        Wout2.reshape(grouped),
    )
```
